```python
import numpy as np

kernel_name = "dist_matmul_relu_kshard_i_m1024_n1024_k512"

def setup_inputs():
    A = np.random.randn(1024, 2048).astype(np.float32)
    B = np.random.randn(2048, 1024).astype(np.float32)
    return {"A": A, "B": B}

def reference(A: np.ndarray, B: np.ndarray) -> np.ndarray:
    z = A @ B
    return np.maximum(z, 0.0)
```

```python
import contextlib
import jax
import jax.numpy as jnp
from jax import lax
from jax.experimental import pallas as pl
from jax.experimental.pallas import tpu as pltpu

M, N, K = 1024, 1024, 512
Q = M // 4
MESH = pl.DeviceIdType.MESH
BF16, F32 = jnp.bfloat16, jnp.float32

P1 = [(0, 128, 0, 128), (128, 128, 0, 128), (0, 256, 128, 128), (0, 256, 256, 256), (0, 256, 512, 512)]
P2 = [(0, 512), (512, 512)]


def pallas_dist_matmul_relu_kshard_i_m1024_n1024_k512_kernel(A, B, scopes=False, P1=P1, P2=P2):
    def scope(n):
        return jax.named_scope(n) if scopes else contextlib.nullcontext()
    n1, n2 = len(P1), len(P2)

    def body(a_hbm, b_hbm, o_ref,
             a32, b32, a16, b16, s1, r1, acc, s2, r2,
             ld_sem, s1_sem, r1_sem, s2_sem, r2_sem, s3_sem, r3_sem):
        me = lax.axis_index("i")
        ybit = (me ^ (me >> 1)) & 1
        xbit = me >> 1
        peer = (me ^ 1, 3 - me)
        bit = (ybit, xbit)
        own_row = [pl.multiple_of((2 * h + bit[h]) * Q, Q) for h in range(2)]
        snd_row = [pl.multiple_of((2 * h + 1 - bit[h]) * Q, Q) for h in range(2)]

        loads, order = {}, []
        def want(key):
            if key not in loads:
                i = len(order)
                if key[0] == "b":
                    _, c0, cn = key
                    cp = pltpu.make_async_copy(b_hbm.at[:, pl.ds(c0, cn)], b32.at[:, pl.ds(c0, cn)], ld_sem.at[i])
                else:
                    _, slot, r0, rn = key
                    row = (snd_row + own_row)[slot]
                    cp = pltpu.make_async_copy(a_hbm.at[pl.ds(row + r0, rn)], a32.at[slot, pl.ds(r0, rn)], ld_sem.at[i])
                loads[key] = cp
                order.append(key)
        have_a = [0, 0]; have_b = 0
        steps = []
        for t, (r0, rn, c0, cn) in enumerate(P1):
            for h in range(2):
                need = []
                if c0 + cn > have_b:
                    need.append(("b", have_b, c0 + cn - have_b)); have_b = c0 + cn
                if r0 + rn > have_a[h]:
                    need.append(("a", h, have_a[h], r0 + rn - have_a[h])); have_a[h] = r0 + rn
                for k in need: want(k)
                steps.append((t, h, need))
        for h in range(2): want(("a", 2 + h, 0, Q))
        for k in order: loads[k].start()

        bar = pltpu.get_barrier_semaphore()
        for p in peer:
            pl.semaphore_signal(bar, inc=1, device_id=(p,), device_id_type=MESH)

        def land(key):
            loads[key].wait()
            if key[0] == "b":
                _, c0, cn = key
                b16[:, pl.ds(c0, cn)] = b32[:, pl.ds(c0, cn)].astype(BF16)
            else:
                _, slot, r0, rn = key
                a16[slot, pl.ds(r0, rn)] = a32[slot, pl.ds(r0, rn)].astype(BF16)

        def mm(slot, r0, rn, c0, cn):
            return jnp.dot(a16[slot, pl.ds(r0, rn)], b16[:, pl.ds(c0, cn)], preferred_element_type=F32)

        def d1(t, h):
            r0, rn, c0, cn = P1[t]
            return pltpu.make_async_remote_copy(
                s1.at[h, pl.ds(r0, rn), pl.ds(c0, cn)], r1.at[h, pl.ds(r0, rn), pl.ds(c0, cn)],
                s1_sem.at[h, t], r1_sem.at[h, t], device_id=(peer[h],), device_id_type=MESH)
        def d2(j, h):
            c0, cn = P2[j]
            return pltpu.make_async_remote_copy(
                s2.at[h, :, pl.ds(c0, cn)], r2.at[h, :, pl.ds(c0, cn)],
                s2_sem.at[h, j], r2_sem.at[h, j], device_id=(peer[1 - h],), device_id_type=MESH)
        def d3(j, h, row):
            c0, cn = P2[j]
            blk = o_ref.at[pl.ds(row, Q), pl.ds(c0, cn)]
            return pltpu.make_async_remote_copy(
                blk, blk, s3_sem.at[h, j], r3_sem.at[h, j], device_id=(peer[h],), device_id_type=MESH)

        for t, h, need in steps:
            with scope(f"p1_{t}{h}"):
                for k in need: land(k)
                r0, rn, c0, cn = P1[t]
                s1[h, pl.ds(r0, rn), pl.ds(c0, cn)] = mm(h, r0, rn, c0, cn).astype(BF16)
                if t == 0 and h == 0:
                    pl.semaphore_wait(bar, 2)
                d1(t, h).start()
        with scope("own"):
            for h in range(2):
                land(("a", 2 + h, 0, Q))
                acc[h] = mm(2 + h, 0, Q, 0, N)
        done1 = set()
        for j, (c0, cn) in enumerate(P2):
            for h in range(2):
                with scope(f"p2_{j}{h}"):
                    for t, (_, _, d0, dn) in enumerate(P1):
                        if d0 < c0 + cn and (t, h) not in done1:
                            d1(t, h).wait_recv(); done1.add((t, h))
                    cols = pl.ds(c0, cn)
                    s2[h, :, cols] = (acc[h, :, cols] + r1[h, :, cols].astype(F32)).astype(BF16)
                    d2(j, h).start()
        for h in range(2):
            for t in range(n1):
                d1(t, h).wait_send()
        for j, (c0, cn) in enumerate(P2):
            for h in range(2):
                with scope(f"p3_{j}{h}"):
                    d2(j, h).wait_recv()
                    cols = pl.ds(c0, cn)
                    z = s2[h, :, cols].astype(F32) + r2[h, :, cols].astype(F32)
                    o_ref[pl.ds(own_row[h], Q), cols] = jnp.maximum(z, 0.0).astype(BF16)
                    d3(j, h, own_row[h]).start()
        with scope("fin_s"):
            for j in range(n2):
                for h in range(2):
                    d2(j, h).wait_send()
            for j in range(n2):
                for h in range(2):
                    d3(j, h, own_row[h]).wait_send()
        with scope("fin_r"):
            for j in range(n2):
                for h in range(2):
                    d3(j, h, snd_row[h]).wait_recv()

    dma = pltpu.SemaphoreType.DMA
    return pl.pallas_call(
        body,
        out_shape=pltpu.VMEM((M, N), BF16),
        in_specs=[pl.BlockSpec(memory_space=pltpu.HBM)] * 2,
        out_specs=pl.BlockSpec(memory_space=pltpu.VMEM),
        scratch_shapes=[
            pltpu.VMEM((4, Q, K), F32), pltpu.VMEM((K, N), F32),
            pltpu.VMEM((4, Q, K), BF16), pltpu.VMEM((K, N), BF16),
            pltpu.VMEM((2, Q, N), BF16), pltpu.VMEM((2, Q, N), BF16),
            pltpu.VMEM((2, Q, N), F32),
            pltpu.VMEM((2, Q, N), BF16), pltpu.VMEM((2, Q, N), BF16),
            dma((3 * n1 + 2,)),
            dma((2, n1)), dma((2, n1)), dma((2, n2)), dma((2, n2)), dma((2, n2)), dma((2, n2)),
        ],
        compiler_params=pltpu.CompilerParams(collective_id=0, vmem_limit_bytes=32 * 2**20),
    )(A, B)
```

```python
import functools

import jax
import jax.numpy as jnp
from jax import lax
from jax.experimental import pallas as pl
from jax.experimental.pallas import tpu as pltpu

M, N, K = 1024, 1024, 512
Q = M // 4
BF16, F32 = jnp.bfloat16, jnp.float32
MESH = pl.DeviceIdType.MESH

TILES = (
    (0, 128, 0, 128),
    (128, 128, 0, 128),
    (0, 256, 128, 128),
    (0, 256, 256, 256),
    (0, 256, 512, 512),
)
CHUNKS = ((0, 512), (512, 512))


def _load_plan():
    steps, loads = [], []
    rows_in, cols_in = [0, 0], 0
    for t, (r0, rn, c0, cn) in enumerate(TILES):
        for k in range(2):
            need = []
            if c0 + cn > cols_in:
                need.append(("b", cols_in, c0 + cn - cols_in))
                cols_in = c0 + cn
            if r0 + rn > rows_in[k]:
                need.append(("a", k, rows_in[k], r0 + rn - rows_in[k]))
                rows_in[k] = r0 + rn
            steps.append((t, k, need))
            loads += need
    loads += [("a", 2 + h, 0, Q) for h in range(2)]
    return steps, loads


def _body(a_hbm, b_hbm, o_ref, a32, b32, a16, b16, s1, r1, acc, s2, r2,
          s3_sem, r3_sem):
    steps, load_keys = _load_plan()
    nt, nc = len(TILES), len(CHUNKS)

    me = lax.axis_index("i")
    xbit = me >> 1
    ybit = (me ^ xbit) & 1
    peer = (me ^ 1, 3 - me)
    bit = (ybit, xbit)
    own_row = [pl.multiple_of((2 * h + bit[h]) * Q, Q) for h in range(2)]
    far_row = [pl.multiple_of((2 * h + 1 - bit[h]) * Q, Q) for h in range(2)]

    def pick(k, pair):
        return jnp.where(xbit == k, pair[0], pair[1])

    lk = [xbit, 1 - xbit]
    lk_peer = [pick(k, peer) for k in range(2)]
    a_row = [pl.multiple_of(pick(k, far_row), Q) for k in range(2)] + own_row

    dma = pltpu.SemaphoreType.DMA

    @functools.partial(
        pl.run_scoped,
        ld_sem=dma((len(load_keys),)),
        s1_sem=dma((2, nt)),
        r1_sem=dma((2, nt)),
        s2_sem=dma((2, nc)),
        r2_sem=dma((2, nc)),
    )
    def _(ld_sem, s1_sem, r1_sem, s2_sem, r2_sem):
        barrier = pltpu.get_barrier_semaphore()
        for p in peer:
            pl.semaphore_signal(barrier, inc=1, device_id=(p,), device_id_type=MESH)

        loads = {}
        for i, key in enumerate(load_keys):
            if key[0] == "b":
                cols = pl.ds(key[1], key[2])
                src, dst = b_hbm.at[:, cols], b32.at[:, cols]
            else:
                _, slot, r0, rn = key
                src = a_hbm.at[pl.ds(a_row[slot] + r0, rn)]
                dst = a32.at[slot, pl.ds(r0, rn)]
            loads[key] = pltpu.make_async_copy(src, dst, ld_sem.at[i])
            loads[key].start()

        def land(key):
            loads[key].wait()
            if key[0] == "b":
                cols = pl.ds(key[1], key[2])
                b16[:, cols] = b32[:, cols].astype(BF16)
            else:
                _, slot, r0, rn = key
                a16[slot, pl.ds(r0, rn)] = a32[slot, pl.ds(r0, rn)].astype(BF16)

        def matmul(slot, r0, rn, c0, cn):
            return jnp.dot(a16[slot, pl.ds(r0, rn)], b16[:, pl.ds(c0, cn)],
                           preferred_element_type=F32)

        def copy1(t, k, h):
            r0, rn, c0, cn = TILES[t]
            rows, cols = pl.ds(r0, rn), pl.ds(c0, cn)
            return pltpu.make_async_remote_copy(
                s1.at[k, rows, cols], r1.at[h, rows, cols],
                s1_sem.at[k, t], r1_sem.at[h, t],
                device_id=(lk_peer[k],), device_id_type=MESH)

        def copy2(j, h):
            cols = pl.ds(*CHUNKS[j])
            return pltpu.make_async_remote_copy(
                s2.at[h, :, cols], r2.at[h, :, cols],
                s2_sem.at[h, j], r2_sem.at[h, j],
                device_id=(peer[1 - h],), device_id_type=MESH)

        def copy3(j, h):
            block = o_ref.at[pl.ds(own_row[h], Q), pl.ds(*CHUNKS[j])]
            return pltpu.make_async_remote_copy(
                block, block, s3_sem.at[h], r3_sem.at[h],
                device_id=(peer[h],), device_id_type=MESH)

        for n, (t, k, need) in enumerate(steps):
            for key in need:
                land(key)
            r0, rn, c0, cn = TILES[t]
            s1[k, pl.ds(r0, rn), pl.ds(c0, cn)] = matmul(k, *TILES[t]).astype(BF16)
            if n == 0:
                pl.semaphore_wait(barrier, 2)
            copy1(t, k, lk[k]).start()

        for h in range(2):
            land(("a", 2 + h, 0, Q))
            acc[h] = matmul(2 + h, 0, Q, 0, N)

        for j, (c0, cn) in enumerate(CHUNKS):
            cols = pl.ds(c0, cn)
            for h in range(2):
                for t, tile in enumerate(TILES):
                    if c0 <= tile[2] < c0 + cn:
                        copy1(t, h, h).wait_recv()
                s2[h, :, cols] = (
                    acc[h, :, cols] + r1[h, :, cols].astype(F32)).astype(BF16)
                copy2(j, h).start()
        for k in range(2):
            for t in range(nt):
                copy1(t, k, k).wait_send()

        for j, (c0, cn) in enumerate(CHUNKS):
            cols = pl.ds(c0, cn)
            for h in range(2):
                copy2(j, h).wait_recv()
                z = s2[h, :, cols].astype(F32) + r2[h, :, cols].astype(F32)
                o_ref[pl.ds(own_row[h], Q), cols] = jnp.maximum(z, 0.0).astype(BF16)
                copy3(j, h).start()
        for j in range(nc):
            for h in range(2):
                copy2(j, h).wait_send()

    quarters = [
        pltpu.make_async_remote_copy(
            o_ref.at[pl.ds(own_row[h], Q)], o_ref.at[pl.ds(far_row[h], Q)],
            s3_sem.at[h], r3_sem.at[h],
            device_id=(peer[h],), device_id_type=MESH)
        for h in range(2)
    ]
    for quarter in quarters:
        quarter.wait_send()
    for quarter in quarters:
        quarter.wait_recv()


def pallas_dist_matmul_relu_kshard_i_m1024_n1024_k512_kernel(
    A: jax.Array,
    B: jax.Array,
):
    return pl.pallas_call(
        _body,
        out_shape=pltpu.VMEM((M, N), BF16),
        in_specs=[pl.BlockSpec(memory_space=pltpu.HBM)] * 2,
        out_specs=pl.BlockSpec(memory_space=pltpu.VMEM),
        scratch_shapes=[
            pltpu.VMEM((4, Q, K), F32),
            pltpu.VMEM((K, N), F32),
            pltpu.VMEM((4, Q, K), BF16),
            pltpu.VMEM((K, N), BF16),
            pltpu.VMEM((2, Q, N), BF16),
            pltpu.VMEM((2, Q, N), BF16),
            pltpu.VMEM((2, Q, N), F32),
            pltpu.VMEM((2, Q, N), BF16),
            pltpu.VMEM((2, Q, N), BF16),
            pltpu.SemaphoreType.DMA((2,)),
            pltpu.SemaphoreType.DMA((2,)),
        ],
        compiler_params=pltpu.CompilerParams(
            collective_id=0, vmem_limit_bytes=32 * 2**20),
    )(A, B)
```
